```python
import numpy as np

kernel_name = "dist_mlp2_tp_i_m512_h1024_out512"

def setup_inputs():
    x = np.random.randn(512, 512).astype(np.float32)
    W1 = np.random.randn(512, 4096).astype(np.float32)
    W2 = np.random.randn(4096, 512).astype(np.float32)
    return {"x": x, "W1": W1, "W2": W2}

def reference(x: np.ndarray, W1: np.ndarray, W2: np.ndarray) -> np.ndarray:
    h = x @ W1
    h = np.maximum(h, 0.0)
    return h @ W2
```

```python
import contextlib

import jax
import jax.numpy as jnp
from jax import lax
from jax.experimental import pallas as pl
from jax.experimental.pallas import tpu as pltpu

L = pl.DeviceIdType.LOGICAL
BF = jnp.bfloat16
F32 = jnp.float32
T = 128


def make(scopes=False):
    def scope(name):
        return jax.named_scope(name) if scopes else contextlib.nullcontext()

    def kernel(x, W1, W2):
        def body(x_hbm, w1_hbm, w2_hbm, out, xv, w1v, w2v, xb, hacc, h, s1, r1, s2, r2,
                 lsem, ssem, rsem):
            me = lax.axis_index("i")
            p = ((me + 1) // 2) % 2
            q = me // 2
            nbr = [me ^ 1, 3 - me]
            bar = pltpu.get_barrier_semaphore()

            loads = []

            def load(src, dst):
                cp = pltpu.make_async_copy(src, dst, lsem.at[len(loads)])
                cp.start()
                loads.append(cp)
                return cp

            lx = load(x_hbm, xv)
            lw1 = []
            for c in range(2):
                for k in range(2):
                    idx = (pl.ds(k * 256, 256), pl.ds(c * 512, 512))
                    lw1.append(load(w1_hbm.at[idx], w1v.at[idx]))
            lw2 = [load(w2_hbm.at[:, pl.ds(c * T, T)], w2v.at[c]) for c in range(4)]
            for n in nbr:
                pl.semaphore_signal(bar, inc=1, device_id=n, device_id_type=L)

            send_rb = [1 - p, 2 + 1 - q]
            keep_rb = [p, 2 + q]
            order = send_rb + keep_rb

            def rows(rb):
                return pl.ds(pl.multiple_of(rb * T, T), T)

            with scope("a_wait_x"):
                lx.wait()
            for i, rb in enumerate(order):
                xb[pl.ds(i * T, T), :] = xv[rows(rb), :].astype(BF)
            for c in range(2):
                cs = pl.ds(c * 512, 512)
                with scope(f"b_wait_w1_{c}0"):
                    lw1[2 * c].wait()
                hacc[...] = jnp.dot(xb[:, 0:256], w1v[0:256, cs].astype(BF),
                                    preferred_element_type=F32)
                with scope(f"b_wait_w1_{c}1"):
                    lw1[2 * c + 1].wait()
                a = hacc[...] + jnp.dot(xb[:, 256:512], w1v[256:512, cs].astype(BF),
                                        preferred_element_type=F32)
                h[:, cs] = jnp.maximum(a, 0.0).astype(BF)

            def rdma(src, dst, k, d):
                return pltpu.make_async_remote_copy(
                    src, dst, ssem.at[k, d], rsem.at[k, d], device_id=nbr[d], device_id_type=L)

            with scope("c_bar"):
                pl.semaphore_wait(bar, 2)
            sends = []
            ph1 = {}
            for c in range(4):
                with scope(f"d_wait_w2_{c}"):
                    lw2[c].wait()
                w = w2v[c].astype(BF)
                s1[c] = jnp.dot(h[0:256, :], w, preferred_element_type=F32).astype(BF)
                for d in range(2):
                    sl = pl.ds(d * T, T)
                    cp = rdma(s1.at[c, sl], r1.at[c, sl], c, d)
                    cp.start()
                    sends.append(cp)
                    ph1[c, d] = cp
                hacc[0:256, pl.ds(c * T, T)] = jnp.dot(h[256:512, :], w, preferred_element_type=F32)
            ph2 = {}
            for c in range(4):
                for d in range(2):
                    sl = pl.ds(d * T, T)
                    with scope(f"e_ph1_{c}{d}"):
                        ph1[c, d].wait_recv()
                    a = hacc[sl, pl.ds(c * T, T)] + r1[c, sl].astype(F32)
                    s2[c, sl] = a.astype(BF)
                    cp = rdma(s2.at[c, sl], r2.at[c, sl], 4 + c, 1 - d)
                    cp.start()
                    sends.append(cp)
                    ph2[c, d] = cp
            ph3 = {}
            for c in range(4):
                for d in range(2):
                    sl = pl.ds(d * T, T)
                    with scope(f"f_ph2_{c}{d}"):
                        ph2[c, d].wait_recv()
                    dst = out.at[rows(keep_rb[d]), pl.ds(c * T, T)]
                    dst[...] = (s2[c, sl].astype(F32) + r2[c, sl].astype(F32)).astype(BF)
                    cp = rdma(dst, dst, 8 + c, d)
                    cp.start()
                    sends.append(cp)
                    land = out.at[rows(send_rb[d]), pl.ds(c * T, T)]
                    ph3[c, d] = rdma(land, land, 8 + c, d)
            for c in range(4):
                for d in range(2):
                    with scope(f"g_ph3_{c}{d}"):
                        ph3[c, d].wait_recv()
            for cp in sends:
                cp.wait_send()

        HBM = pl.BlockSpec(memory_space=pltpu.MemorySpace.HBM)
        return pl.pallas_call(
            body,
            out_shape=jax.ShapeDtypeStruct((512, 512), BF),
            in_specs=[HBM] * 3,
            out_specs=pl.BlockSpec(memory_space=pltpu.MemorySpace.VMEM),
            scratch_shapes=[
                pltpu.VMEM((512, 512), F32),
                pltpu.VMEM((512, 1024), F32),
                pltpu.VMEM((4, 1024, T), F32),
                pltpu.VMEM((512, 512), BF),
                pltpu.VMEM((512, 512), F32),
                pltpu.VMEM((512, 1024), BF),
                pltpu.VMEM((4, 256, T), BF),
                pltpu.VMEM((4, 256, T), BF),
                pltpu.VMEM((4, 256, T), BF),
                pltpu.VMEM((4, 256, T), BF),
                pltpu.SemaphoreType.DMA((9,)),
                pltpu.SemaphoreType.DMA((12, 2)),
                pltpu.SemaphoreType.DMA((12, 2)),
            ],
            compiler_params=pltpu.CompilerParams(collective_id=0, disable_semaphore_checks=True),
        )(x, W1, W2)

    return kernel


def pallas_dist_mlp2_tp_i_m512_h1024_out512_kernel(x, W1, W2):
    return make()(x, W1, W2)
```

```python
import re

import jax
import jax.numpy as jnp
from jax import lax
from jax.experimental import pallas as pl
from jax.experimental.pallas import tpu as pltpu

SCHEDULE = {
    "M": """
Lx013u Lp0123 Lc01 Wx013u enter x>:03u1 xA:4 x>:4
Wp01 k01:014 fence
Wp2 k2:014 fence xA:5 x>:5l
xC:2 k012:25 fence
Wp3 xC:3l k3:01245 h01234567:3
xA:6 h01234567:6 Lc2 fence
Wc0 c0:0 ^c0:14 rawA:0.0
^c0:256 rawC:4.0 rawA:1.0 xA:7
^h012345:7 rawC:56.0 rawA:2.0 xC:a
h67:7 c0:3 c0:7 Lc3 ^h0123:a rawA:3.0 rawC:7.0 Wc1
c1:0 ^c1:14 rawA:0.1
^c1:256 rawC:4.1 rawA:1.1
^c1:37 ^h45:a rawC:56.1 rawA:2.1 xC:blbu xA:9
h0123:b h01:9 h67:a Lxcdef ^h4567:b rawA:3.1 rawC:7.1 Wc2
c2:0 ^c2:14 rawA:0.2
^c2:235 rawC:4.2 rawA:1.2
^h234567:9 rawC:5.2,3.2 rawA:2.2 xC:8
h01:8 c2:6 c0:a ^h2345:8 ^c2:7 rawC:6.2 relayA:2.0
c0:b ^h67:8 ^c0:9 ^c1:b rawC:7.2 relayA:3.0 Wc3
c3:0 ^c1:a ^c3:1 rawC:0.3 relayA:1.0
c0:8 ^c1:89 ^c3:2 rawC:1.3 relayA:0.0
^c2:89 ^c3:3 rawC:2.3 relayA:2.1 Wxcdef
^h0123:c ^c3:4 rawC:3.3 relayA:3.1
^h4567:c ^c3:5 rawC:4.3 relayA:1.1
^h01:d ^c2:a ^c3:6 rawC:5.3 relayA:0.1
^h2345:d ^c3:7 rawC:6.3 relayA:0.2
^h67:d ^h01:f ^c0:c rawC:7.3 relayA:1.2 <A:4567.01
^h0123:e ^c1:c relayC:4.0 relayA:2.2 <A:4567.23
^h4567:e ^c0:d relayC:4.1 relayA:4.0
^h2345:f ^c1:d relayC:5.0 relayA:4.1
^c2:cde relayC:5.1 relayA:5.0
^h67:f ^c0:e ^c2:b relayC:6.2 relayA:5.1 <A:3.23
^c3:89 ^c1:e relayC:6.0 relayA:4.2
^c3:cde relayC:6.1 relayA:5.2
^c012:f relayC:4.3 relayA:3.2
^c3:abf relayC:56.3 relayA:6.0
relayC:7.0123,3.3 relayA:6.12 relayC:012.3 relayA:0.3,1.3 relayC:345.2
relayA:2.3,3.3,4.3 relayC:0123.0 relayA:5.3,7.01 relayC:0123.1 relayA:7.2,6.3,7.3 relayC:012.2
""",
    "C": """
Lx2 Lx3l Lp0123 Lc01 Wx2 enter x>:2 Wx3l x>:3labl xM:0
Wp01 k01:02 fence xM:3u x>:bu8
Wp2 k2:02 k012:3 fence
xM:1 k012:1
Wp3 k3:0123 Lc2 Lx5u fence
Wc0 c0:2 ^c0:3 term:2.0
^c0:0l1 term:3.0 xM:4
c0:0u Lc3 ^h012:4 term:1.0,0.0
h3:4 fence
Wc1 c1:2 ^c1:3 term:2.1
^c1:0l1 term:3.1 xM:5l
c1:0u Lx67 ^h456:4 term:1.1,0.1
h7:4 fence
Wc2 c2:0 ^c2:12l term:0.2 <M:4.0 Wx5u
c2:2u ^h012:5 term:1.2,2.2 <M:4.1
h345:5 c0:4 ^h67:5 ^c1:4l term:4.0 <M:567.0,5.1
c1:4u ^c2:4 term:4.1 <M:4.2
c0:5 ^c1:5 ^c2:5l term:5.0 <M:5.2
c2:5u ^c2:3 term:5.1,4.2,5.2 Wc3 Wx67 <M:3.2
h01234567:6 ^h01:7 term:3.2 <M:6.2,7.12
c0:6 ^c1:6 ^c2:6l term:6.0
c2:6u ^h23:7 ^c3:0l term:6.12 <M:01.3
c3:0u1 ^h45:7 ^c3:2l term:0.3,1.3 <M:23.3
c3:2u3 ^h67:7 ^c3:4l term:2.3,3.3 <M:45.3
c3:4u5 ^c3:6 term:4.3,5.3
c0123:7 term:7.012,6.3,7.3
final:6.201,4.3,56.3,7.0123,3.3,012.3
""",
    "A": """
Lx14567 Lp0123 Lc01 Wx14567 enter x>:45679
Wp01 k01:14567
Wp2 k2:14567 fence
Wp3 k3:14567 Lc2 fence
Wc0 c0:45 ^c0:1 term:45.0
c0:67 Lc3 term:67.0
Wc1 c1:45 ^c1:1 term:45.1
c1:67 Lx023 term:67.1
Wc2 c2:45 ^c2:1 term:45.2
c2:67 term:67.2
Wc3 c3:45 ^c3:1 term:45.3
c3:67 term:67.3,1.3,1.0
Wx023 h01234567:3 h01:02 c23:3 ^h2:02 term:3.23,1.1 <M:023.01
h345:02 c01:3 ^h6:02 term:3.01
h7:02 c3:02 term:02.3,1.2 <M:02.2
c0:02 ^c1:0 term:02.0
c1:2 c2:02 term:02.12
final:0123.01,012.2,45.012,3.2
""",
}

M, K, H, N = 512, 512, 1024, 512
LANES = 128
HALF = M // 2
HEAD = 8
W2_RUN = 64


def _pieces(text):
    return [
        (32 * int(g, 16) + 16 * (half == "u"), 16 if half else 32)
        for g, half in re.findall("([0-9a-f])([lu]?)", text)
    ]


def _joined(pieces):
    runs = []
    for r, n in sorted(pieces):
        if runs and sum(runs[-1]) == r != HALF:
            runs[-1] = (runs[-1][0], runs[-1][1] + n)
        else:
            runs.append((r, n))
    return runs


def _tiles(text):
    return [
        (r, n, int(c))
        for part in text.split(",")
        for c in part.split(".")[1]
        for r, n in _joined(_pieces(part.split(".")[0]))
    ]


def _cells(r, n, c):
    return [(row, c) for row in range(r, r + n, 16)]


def _shifted(r):
    return (r + HALF) % M


def _transfers(schedule):
    links = {("A", "M"): [], ("C", "M"): [], ("M", "A"): [], ("M", "C"): []}
    for role, text in schedule.items():
        for op, _, arg in (word.partition(":") for word in text.split()):
            if op == "x>":
                links[role, "C" if role == "M" else "M"] += [("x", r, n, None) for r, n in _pieces(arg)]
            elif op in ("term", "final"):
                links[role, "M"] += [(op, *tile) for tile in _tiles(arg)]
            elif op[:-1] in ("raw", "relay"):
                links[role, op[-1]] += [(op[:-1], *tile) for tile in _tiles(arg)]
    return links


class _Chip:
    def __init__(self, role, position, links, totals, refs):
        self.role, self.links = role, links
        self.totals = totals
        (self.x_hbm, self.w1_hbm, self.w2_hbm, self.out, self.x_f32, self.w1, self.w2, self.x,
         self.pre, self.h, self.own, self.sums, self.inbox,
         self.load_sems, self.send_sems, self.recv_sems, self.fence_sem) = refs
        self.middle = role == "M"
        self.peers = (0, 2) if self.middle else (1, 3)
        self.side = lax.shift_right_logical(position, 1) if self.middle else "AC".index(role)
        self.loads = {"p0": []}
        self.sends = []
        self.arrived = set()
        self.quarters = {}
        self.summed = {}
        self.complete = set()

    def out_rows(self, r, n):
        if not self.middle:
            return pl.ds(r, n)
        shift = (1 - self.side) * HALF
        return pl.ds(pl.multiple_of(r + shift if r < HALF else r - shift, 16), n)

    def out_tile(self, r, n, c):
        return self.out.at[self.out_rows(r, n), pl.ds(c * LANES, LANES)]

    def rows(self, text):
        pieces = _pieces(text)
        return pieces if self.middle else pieces + [(r + HALF, n) for r, n in pieces]

    def load(self, name):
        waits = self.loads.setdefault(name, [])
        sem = self.load_sems.at[list(self.loads).index(name)]
        if name[0] == "x":
            for r, n in _joined(self.rows(name[1:])):
                waits.append(pltpu.make_async_copy(
                    self.x_hbm.at[self.out_rows(r, n)], self.x_f32.at[pl.ds(r, n)], sem))
                waits[-1].start()
            return
        i = int(name[1])
        if name[0] == "p":
            first = max(i * LANES, HEAD)
            rows = pl.ds(first, (i + 1) * LANES - first)
            pltpu.make_async_copy(self.w1_hbm.at[rows], self.w1.at[rows, pl.ds(0, H)], sem).start()
            whole = self.w1.at[pl.ds(i * LANES, LANES), pl.ds(0, H)]
        else:
            whole = self.w2[i]
            for j in range(0, W2_RUN, 8):
                pltpu.make_async_copy(
                    self.w2_hbm.at[:, pl.ds(j, 8), pl.ds(i * LANES, LANES)],
                    whole.at[:, pl.ds(j, 8)], sem).start()
        waits.append(pltpu.make_async_copy(whole, whole, sem))

    def wait_load(self, name):
        for copy in self.loads[name]:
            copy.wait()
        if name[0] == "x":
            for r, n in _joined(self.rows(name[1:])):
                self.x[pl.ds(r, n), :] = self.x_f32[pl.ds(r, n), :].astype(jnp.bfloat16)

    def hidden(self, by_rows, blocks, text):
        runs = _joined(self.rows(text))
        span = pl.ds(blocks[0] * LANES, len(blocks) * LANES)
        ks, cols = (span, pl.ds(0, H)) if by_rows else (pl.ds(0, K), span)
        lhs = jnp.concatenate([self.x[pl.ds(r, n), ks] for r, n in runs], axis=0)
        value = jnp.dot(lhs, self.w1[ks, cols].astype(jnp.bfloat16), preferred_element_type=jnp.float32)

        def store():
            at = 0
            for r, n in runs:
                v, at = value[at:at + n], at + n
                before = self.quarters.get(r, 0)
                if by_rows:
                    self.quarters.update((row, before + len(blocks)) for row in range(r, r + n, 16))
                if before:
                    v = v + self.pre[pl.ds(r, n), cols]
                if by_rows and before + len(blocks) < K // LANES:
                    self.pre[pl.ds(r, n), cols] = v
                else:
                    self.h[pl.ds(r, n), cols] = jnp.maximum(v, 0.0).astype(jnp.bfloat16)

        return store

    def output(self, c, text):
        pieces = self.rows(text)
        lhs = jnp.concatenate([self.h[pl.ds(r, n), :] for r, n in pieces], axis=0)
        rhs = self.w2[c][...].reshape(H, LANES).astype(jnp.bfloat16)
        value = jnp.dot(lhs, rhs, preferred_element_type=jnp.float32)

        def store():
            at = 0
            for r, n in pieces:
                v, at = value[at:at + n], at + n
                cell = (r % HALF, c)
                if self.middle and r < HALF:
                    self.put_sum(0 if self.carrier("M", "A", "raw", cell) else 1, r, n, c, v)
                elif self.middle:
                    got = [link for link in (0, 1)
                           if ("AC"[link], self.carrier("AC"[link], "M", "term", cell)) in self.arrived]
                    if len(got) == 1:
                        self.put_sum(1 - got[0], r, n, c, v + self.received(got[0], r, n, c))
                    else:
                        self.own[c, pl.ds(r, n)] = v
                else:
                    raw = self.carrier("M", self.role, "raw", cell)
                    if raw is None:
                        self.put_sum(0, r, n, c, v)
                    elif ("M", raw) in self.arrived:
                        self.put_sum(0, r, n, c, v + self.received(int(r < HALF), r, n, c))
                    else:
                        self.own[c, pl.ds(r, n)] = v

        return store

    def put_sum(self, index, r, n, c, value):
        self.sums[index][c, pl.ds(r, n)] = value.astype(jnp.bfloat16)
        self.summed.update((cell, index) for cell in _cells(r, n, c))

    def received(self, link, r, n, c):
        return self.inbox[link, c, pl.ds(r, n)].astype(jnp.float32)

    def put_total(self, index, link, r, n, c):
        value = self.sums[index][c, pl.ds(r, n)].astype(jnp.float32) + self.received(link, r, n, c)
        self.out_tile(r, n, c)[...] = value.astype(jnp.bfloat16)

    def carrier(self, sender, receiver, kind, cell):
        return next((t for t in self.links[sender, receiver] if t[0] == kind and cell in _cells(*t[1:])), None)

    def routes(self, peer, transfer):
        kind, r, _, _ = transfer
        row = r + HALF if kind in ("term", "relay") else r
        if self.middle:
            return [("AC".index(peer), row, row)]
        return [(0, _shifted(row), row), (1, row, row)]

    def remote(self, src, dst, send_sem, recv_slot, link):
        return pltpu.make_async_remote_copy(
            src, dst, send_sem, self.recv_sems.at[recv_slot],
            device_id=self.peers[link], device_id_type=pl.DeviceIdType.LOGICAL)

    def send(self, peer, transfer):
        kind, _, n, c = transfer
        slot = self.side * (self.recv_sems.shape[0] // 2) + self.links[self.role, peer].index(transfer)
        for link, here, at_middle in self.routes(peer, transfer):
            there = self.out_rows(here, n) if self.middle else pl.ds(at_middle, n)
            if kind == "x":
                src, dst = self.x.at[pl.ds(here, n)], self.x.at[there]
            elif kind == "final" or (peer, transfer) in self.totals:
                src = dst = self.out_tile(here, n, c)
            else:
                src = self.sums[self.summed[here, c]].at[c, pl.ds(here, n)]
                dst = self.inbox.at[self.side, c, there]
            self.sends.append(self.remote(src, dst, self.send_sems.at[len(self.sends)], slot, link))
            self.sends[-1].start()

    def receive(self, peer, transfer):
        if (peer, transfer) in self.arrived:
            return
        self.arrived.add((peer, transfer))
        kind, _, n, c = transfer
        total = kind == "final" or (self.role, transfer) in self.totals
        routes = self.routes(peer, transfer)
        for link, here, _ in routes:
            if kind == "x":
                dst = self.x.at[pl.ds(here, n)]
            else:
                dst = self.out_tile(here, n, c) if total else self.inbox.at[link, c, pl.ds(here, n)]
            slot = link * (self.recv_sems.shape[0] // 2) + self.links[peer, self.role].index(transfer)
            self.remote(dst, dst, self.send_sems.at[0], slot, link).wait_recv()
        if kind == "relay" and not total:
            for link, here, _ in routes:
                self.put_total(0, link, here, n, c)

    def receive_tile(self, peer, kind, tile):
        for cell in _cells(*tile):
            transfer = self.carrier(peer, self.role, kind, cell)
            if transfer:
                self.receive(peer, transfer)

    def relay(self, end, tile):
        near = "AC".index(end)
        self.receive_tile("CA"[near], "term", tile)
        total = all((end, self.carrier(end, "M", "term", cell)) in self.arrived for cell in _cells(*tile))
        for r, c in _cells(tile[0] + HALF, *tile[1:]):
            if (r, c) not in self.summed:
                self.put_sum(near, r, 16, c, self.own[c, pl.ds(r, 16)] + self.received(1 - near, r, 16, c))
            assert total or self.summed[r, c] == near
            if total and (r, c) not in self.complete:
                self.complete.add((r, c))
                self.put_total(self.summed[r, c], self.summed[r, c], r, 16, c)
        if total:
            self.totals.add((end, ("relay", *tile)))
        self.send(end, ("relay", *tile))

    def term(self, tile):
        self.receive_tile("M", "raw", tile)
        for row, c in _cells(*tile):
            for link, r in ((1, row), (0, row + HALF)):
                if (r, c) not in self.summed:
                    self.put_sum(0, r, 16, c, self.own[c, pl.ds(r, 16)] + self.received(link, r, 16, c))
        self.send("M", ("term", *tile))

    def fence(self):
        pl.semaphore_signal(self.fence_sem, 1)
        pl.semaphore_wait(self.fence_sem, 1)

    def run(self, text):
        barrier = pltpu.get_barrier_semaphore()
        for peer in self.peers:
            pl.semaphore_signal(barrier, 1, device_id=peer, device_id_type=pl.DeviceIdType.LOGICAL)
        started = []
        for line in text.strip().splitlines():
            for store in started:
                store()
            started = []
            for word in line.split():
                op, _, arg = word.lstrip("^").partition(":")
                if op[0] in "LW":
                    for name in [op[1:]] if op[1] == "x" else [op[1] + i for i in op[2:]]:
                        (self.load if op[0] == "L" else self.wait_load)(name)
                elif op == "enter":
                    pl.semaphore_wait(barrier, 2)
                elif op == "fence":
                    self.fence()
                elif op[0] in "khc":
                    blocks = [int(i) for i in op[1:]]
                    stores = ([self.output(c, arg) for c in blocks] if op[0] == "c"
                              else [self.hidden(op[0] == "k", blocks, arg)])
                    if word[0] == "^":
                        started += stores
                    else:
                        for store in stores:
                            store()
                elif op[0] == "x":
                    for r, n in _pieces(arg):
                        if op == "x>":
                            self.send("C" if self.middle else "M", ("x", r, n, None))
                        else:
                            self.receive(op[1], ("x", r, n, None))
                else:
                    for tile in _tiles(arg):
                        if op[0] == "<":
                            self.receive_tile(op[1], "term" if self.middle else "raw", tile)
                        elif op == "term":
                            self.term(tile)
                        elif op == "final":
                            self.receive_tile("M", "relay", tile)
                            self.send("M", ("final", *tile))
                        elif op[:-1] == "raw":
                            self.send(op[-1], ("raw", *tile))
                        else:
                            self.relay(op[-1], tile)
        assert not started
        rest = [(sender, t) for sender, receiver in self.links if receiver == self.role
                for t in self.links[sender, receiver] if (sender, t) not in self.arrived]
        for copy in self.sends[:-8]:
            copy.wait_send()
        self.fence()
        for sender, transfer in rest[:-1]:
            self.receive(sender, transfer)
        self.fence()
        for copy in self.sends[-8:]:
            copy.wait_send()
        self.fence()
        self.receive(*rest[-1])


def _mlp(schedule, x, W1, W2):
    links = _transfers(schedule)

    def body(*refs):
        w1_hbm, w1, load_sems = refs[1], refs[5], refs[-4]
        head = pl.ds(0, HEAD)
        pltpu.make_async_copy(w1_hbm.at[head], w1.at[head, pl.ds(0, H)], load_sems.at[0]).start()
        position = lax.axis_index("i")
        totals = set()
        for role, mine in (("M", (position & 1) == 1), ("C", position == 2), ("A", position == 0)):
            pl.when(mine)(lambda role=role: _Chip(role, position, links, totals, refs).run(schedule[role]))

    longest = max(len(transfers) for transfers in links.values())
    blocks = N // LANES
    hbm = pl.BlockSpec(memory_space=pltpu.MemorySpace.HBM)
    return pl.pallas_call(
        body,
        out_shape=jax.ShapeDtypeStruct((M, N), jnp.bfloat16),
        in_specs=[hbm, hbm, hbm],
        out_specs=pl.BlockSpec(memory_space=pltpu.MemorySpace.VMEM),
        scratch_shapes=[
            pltpu.VMEM((M, K), jnp.float32),
            pltpu.VMEM((K, H + LANES), jnp.float32),
            [pltpu.VMEM((H // W2_RUN, W2_RUN, LANES), jnp.float32)] * blocks,
            pltpu.VMEM((M, K), jnp.bfloat16),
            pltpu.VMEM((M, H + LANES), jnp.float32),
            pltpu.VMEM((M, H), jnp.bfloat16),
            pltpu.VMEM((blocks, M, LANES), jnp.float32),
            [pltpu.VMEM((blocks, M, LANES), jnp.bfloat16)] * 2,
            pltpu.VMEM((2, blocks, M, LANES), jnp.bfloat16),
            pltpu.SemaphoreType.DMA((12,)),
            pltpu.SemaphoreType.DMA((2 * longest,)),
            pltpu.SemaphoreType.DMA((2 * longest,)),
            pltpu.SemaphoreType.REGULAR,
        ],
        compiler_params=pltpu.CompilerParams(
            collective_id=0,
            disable_bounds_checks=True,
            disable_semaphore_checks=True,
            flags={"XLA_TPU_RESCHEDULE_DMA_DONES": True},
        ),
    )(x, W1, W2.reshape(H // W2_RUN, W2_RUN, N))


def pallas_dist_mlp2_tp_i_m512_h1024_out512_kernel(
    x: jax.Array,
    W1: jax.Array,
    W2: jax.Array,
):
    return _mlp(SCHEDULE, x, W1, W2)
```

```python
import re

import jax
import jax.numpy as jnp
from jax import lax
from jax.experimental import pallas as pl
from jax.experimental.pallas import tpu as pltpu

SCHEDULE = {
    "M": """
Lx01 Lp0123 Lc01 Wx01 enter x>:01 xA:3u x>:3u
Wp01 k01:01 fence xA:4 x>:4
k01:4 Wp2 k2:014 fence xA:5l x>:5l
xC:2 k012:23u5l fence xA:5u x>:5u
Wp3 xC:3l k3:0123u45l h01234567:3l5u
xA:6l xC:al h01234567:6lal Lc2 fence
Wc0 c0:0 ^c0:14 rawA:0.0
^c0:23l56l rawC:4.0 rawA:1.0 xA:6u7l
^h012345:6u7l rawC:56l.0 rawA:23l.0 xC:aubl
h67:6u7l c0:3u6u7l Lc3 ^h0123:aubl rawC:6u7l.0 rawA:3u.0 Wc1
c1:0l4l ^c1:0u1l4u5l rawA:0l.1 rawC:4l.1
^c1:1u25u6 rawA:0u1l.1 rawC:4u5l.1 xA:7u9l
^h012345:7u9l rawC:5u6.1 rawA:1u2.1 xC:8
h67:7u9l h4:aubl c1:3 c1:7 Lxcdef ^h567:aubl ^h0:8 rawC:7.1 rawA:3.1 Wc2
c2:0l4l ^c2:0u1l4u5l rawA:0l.2 rawC:4l.2
^c2:1u235u rawA:0u1l.2 rawC:4u5l.2
^h123456:8 rawC:5u.2,3.2 rawA:1u2.2 xC:bu9u
h7:8 c2:6 c0:7ua ^h0123:9ubu ^c2:7 rawC:6.2,7u.0 relayA:2.0
c0:8 ^h4567:9ubu ^c1:a rawC:7.2 relayA:0.0 Wc3
c3:0 c0:b ^c0:9 ^c1:b ^c3:1 rawC:0.3 relayA:3.0
^c1:89 ^c3:2 rawC:1.3 relayA:1.0
^c2:89 ^c3:3 rawC:2.3 relayA:2.1 Wxcdef
^h0123:c ^c3:4 rawC:3.3 relayA:3.1
^h4567:c ^c3:5 rawC:4.3 relayA:1.1
^c2:a ^c3:9 ^c3:6 rawC:5.3 relayA:0.1
^h0123:d ^c3:7 rawC:6.3 relayA:0.2
^h4567:d ^c0:c rawC:7.3 relayA:1.2 <A:4567.01
^h0123:e ^c1:c relayC:4.0 relayA:2.2 <A:4567.23
^h4567:e ^c0:d relayC:4.1 relayA:4.0
^h0123:f ^c1:d relayC:5.0 relayA:4.1
^c2:cde relayC:5.1 relayA:5.0
^h45:f ^c0:e ^c2:b relayC:6.2 relayA:5.1 <A:3.23
^h67:f ^c3:8 ^c1:e relayC:6.0 relayA:4.2
^c3:cde relayC:6.1,3u.2 relayA:5.2
^c012:f relayC:4.3 relayA:3.2
^c3:abf relayC:56.3 relayA:6.0
relayC:7.0123,3.3 relayA:6.12 relayC:012.3 relayA:0.3,1.3 relayC:3l45.2
relayA:2.3,3.3,4.3 relayC:0123.0 relayA:5.3,7.01 relayC:0123.1 relayA:7.2,6.3,7.3 relayC:012.2
""",
    "C": """
Lx2 Lx3l Lp0123 Lc01 Wx2 enter x>:2 Wx3l x>:3lalaubl xM:0 x>:8
Wp01 k01:02 fence
Wp2 k2:02
xM:1 k012:1 fence xM:3u x>:bu9u
k012:3
Wp3 k3:0123 Lc2 fence
Wc0 c0:2l ^c0:0l2u term:2l.0
^c0:0u3 term:2u.0,0l.0 xM:4
^h012:4 term:0u.0,3.0
c0:1 h3:4 Lc3 ^h45:4 term:1.0 Wc1
c1:2l ^c1:2u3l term:2l.1
^c1:3u1 term:2u.1,3l.1 xM:5l5u
^h67:4 ^h0:5 term:3u.1,1.1
c1:0 h1:5 Lx67 ^h23:5 term:0.1 Wc2
c2:0l ^c2:0u1l term:0l.2
^c2:1u2 term:0u.2,1l.2 <M:45.0,4.1
^h456:5 term:1u.2,2.2
h7:5 c0:4 ^c1:4 ^c2:4l term:4.0 <M:5.1
^c0:5 ^c2:4u term:4.1
c1:5 ^c2:5 ^c2:3l term:5.01,4.2 Wc3 Wx67
c2:3u ^h012:6 term:5.2,3.2 <M:6.01,7.1
h34567:6 h01:7 c0:6 ^c1:6 ^c2:6l term:6.0 <M:67.2
c2:6u ^h23:7 ^c3:0l term:6.12 <M:01.3,7.0
c3:0u1 ^h45:7 ^c3:2l term:0.3,1.3 <M:23.3
c3:2u3 ^h67:7 ^c3:4l term:2.3,3.3 <M:45.3
c3:4u5 ^c3:6 term:4.3,5.3
c0123:7 term:7.012,6.3,7.3
final:6.201,3u.2,4.3,56.3,7.0123,3.3,012.3
""",
    "A": """
Lx13u4567 Lp0123 Lc01 Wx13u4567 enter x>:3u45l5u6l6u7l7u9l
Wp01 k01:14567
Wp2 k2:14567 fence
Wp3 k3:14567 Lc2 fence
Wc0 c0:45 ^c0:1 term:45.0
c0:67 Lc3 term:67.0
Wc1 c1:45 ^c1:1 term:45.1
c1:67 Lx023l term:67.1
Wc2 c2:45 ^c2:1 term:45.2
c2:67 term:67.2
Wc3 c3:45 ^c3:1 term:45.3
c3:67 term:67.3,1.3,1.0
Wx023l h01234567:3 h01:02 c23:3 ^h2:02 term:3.23,1.1 <M:023.01
h345:02 c01:3 ^h6:02 term:3.01
h7:02 c3:02 term:02.3,1.2 <M:02.2
c0:02 ^c1:0 term:02.0
c1:2 c2:02 term:02.12
final:0123.01,012.2,45.012,3l.2
""",
}

M, K, H, N = 512, 512, 1024, 512
LANES = 128
HALF = M // 2
CELL = 16
HEAD = 8
W2_RUN = 64


def _pieces(text):
    return [
        (32 * int(g, 16) + 16 * (half == "u"), 16 if half else 32)
        for g, half in re.findall("([0-9a-f])([lu]?)", text)
    ]


def _joined(pieces):
    runs = []
    for r, n in sorted(pieces):
        if runs and sum(runs[-1]) == r != HALF:
            runs[-1] = (runs[-1][0], runs[-1][1] + n)
        else:
            runs.append((r, n))
    return runs


def _tiles(text):
    return [
        (r, n, int(c))
        for part in text.split(",")
        for c in part.split(".")[1]
        for r, n in _joined(_pieces(part.split(".")[0]))
    ]


def _cells(r, n, c):
    return [(row, c) for row in range(r, r + n, CELL)]


def _shifted(r):
    return (r + HALF) % M


def _transfers(schedule):
    links = {("A", "M"): [], ("C", "M"): [], ("M", "A"): [], ("M", "C"): []}
    for role, text in schedule.items():
        for op, _, arg in (word.partition(":") for word in text.split()):
            if op == "x>":
                links[role, "C" if role == "M" else "M"] += [("x", r, n, None) for r, n in _pieces(arg)]
            elif op in ("term", "final"):
                links[role, "M"] += [(op, *tile) for tile in _tiles(arg)]
            elif op[:-1] in ("raw", "relay"):
                links[role, op[-1]] += [(op[:-1], *tile) for tile in _tiles(arg)]
    return links


class _Chip:
    def __init__(self, role, position, links, totals, refs):
        self.role, self.links = role, links
        self.totals = totals
        (self.x_hbm, self.w1_hbm, self.w2_hbm, self.out, self.x_f32, self.w1, self.w2, self.x,
         self.pre, self.h, self.own, self.sums, self.inbox,
         self.load_sems, self.send_sems, self.recv_sems, self.fence_sem) = refs
        self.middle = role == "M"
        self.peers = (0, 2) if self.middle else (1, 3)
        self.side = lax.shift_right_logical(position, 1) if self.middle else "AC".index(role)
        self.loads = {"p0": []}
        self.sends = []
        self.arrived = set()
        self.quarters = {}
        self.summed = {}
        self.complete = set()

    def out_rows(self, r, n):
        if not self.middle:
            return pl.ds(r, n)
        shift = (1 - self.side) * HALF
        return pl.ds(pl.multiple_of(r + shift if r < HALF else r - shift, CELL), n)

    def out_tile(self, r, n, c):
        return self.out.at[self.out_rows(r, n), pl.ds(c * LANES, LANES)]

    def rows(self, text):
        pieces = _pieces(text)
        return pieces if self.middle else pieces + [(r + HALF, n) for r, n in pieces]

    def load(self, name):
        waits = self.loads.setdefault(name, [])
        sem = self.load_sems.at[list(self.loads).index(name)]
        if name[0] == "x":
            for r, n in _joined(self.rows(name[1:])):
                waits.append(pltpu.make_async_copy(
                    self.x_hbm.at[self.out_rows(r, n)], self.x_f32.at[pl.ds(r, n)], sem))
                waits[-1].start()
            return
        i = int(name[1])
        if name[0] == "p":
            first = max(i * LANES, HEAD)
            rows = pl.ds(first, (i + 1) * LANES - first)
            pltpu.make_async_copy(self.w1_hbm.at[rows], self.w1.at[rows, pl.ds(0, H)], sem).start()
            whole = self.w1.at[pl.ds(i * LANES, LANES), pl.ds(0, H)]
        else:
            whole = self.w2[i]
            for j in range(0, W2_RUN, 8):
                pltpu.make_async_copy(
                    self.w2_hbm.at[:, pl.ds(j, 8), pl.ds(i * LANES, LANES)],
                    whole.at[:, pl.ds(j, 8)], sem).start()
        waits.append(pltpu.make_async_copy(whole, whole, sem))

    def wait_load(self, name):
        for copy in self.loads[name]:
            copy.wait()
        if name[0] == "x":
            for r, n in _joined(self.rows(name[1:])):
                self.x[pl.ds(r, n), :] = self.x_f32[pl.ds(r, n), :].astype(jnp.bfloat16)

    def hidden(self, by_rows, blocks, text):
        runs = _joined(self.rows(text))
        span = pl.ds(blocks[0] * LANES, len(blocks) * LANES)
        ks, cols = (span, pl.ds(0, H)) if by_rows else (pl.ds(0, K), span)
        lhs = jnp.concatenate([self.x[pl.ds(r, n), ks] for r, n in runs], axis=0)
        value = jnp.dot(lhs, self.w1[ks, cols].astype(jnp.bfloat16), preferred_element_type=jnp.float32)

        def store():
            at = 0
            for r, n in runs:
                v, at = value[at:at + n], at + n
                before = self.quarters.get(r, 0)
                if by_rows:
                    self.quarters.update((row, before + len(blocks)) for row in range(r, r + n, CELL))
                if before:
                    v = v + self.pre[pl.ds(r, n), cols]
                if by_rows and before + len(blocks) < K // LANES:
                    self.pre[pl.ds(r, n), cols] = v
                else:
                    self.h[pl.ds(r, n), cols] = jnp.maximum(v, 0.0).astype(jnp.bfloat16)

        return store

    def output(self, c, text):
        pieces = self.rows(text)
        lhs = jnp.concatenate([self.h[pl.ds(r, n), :] for r, n in pieces], axis=0)
        rhs = self.w2[c][...].reshape(H, LANES).astype(jnp.bfloat16)
        value = jnp.dot(lhs, rhs, preferred_element_type=jnp.float32)

        def store():
            for i, r in enumerate(r for piece in pieces for r, _ in _cells(*piece, c)):
                v, cell = value[i * CELL:(i + 1) * CELL], (r % HALF, c)
                if self.middle and r < HALF:
                    self.put_sum(0 if self.carrier("M", "A", "raw", cell) else 1, r, c, v)
                elif self.middle:
                    got = [link for link, end in enumerate("AC")
                           if (end, self.carrier(end, "M", "term", cell)) in self.arrived]
                    if got:
                        self.put_sum(1 - got[0], r, c, v + self.received(got[0], r, c))
                    else:
                        self.own[c, pl.ds(r, CELL)] = v
                else:
                    raw = self.carrier("M", self.role, "raw", cell)
                    if raw is None:
                        self.put_sum(0, r, c, v)
                    elif ("M", raw) in self.arrived:
                        self.put_sum(0, r, c, v + self.received(int(r < HALF), r, c))
                    else:
                        self.own[c, pl.ds(r, CELL)] = v

        return store

    def put_sum(self, index, r, c, value):
        self.sums[index][c, pl.ds(r, CELL)] = value.astype(jnp.bfloat16)
        self.summed[r, c] = index

    def received(self, link, r, c):
        return self.inbox[link, c, pl.ds(r, CELL)].astype(jnp.float32)

    def put_total(self, link, r, c):
        value = self.sums[self.summed[r, c]][c, pl.ds(r, CELL)].astype(jnp.float32) + self.received(link, r, c)
        self.out_tile(r, CELL, c)[...] = value.astype(jnp.bfloat16)

    def carrier(self, sender, receiver, kind, cell):
        return next((t for t in self.links[sender, receiver] if t[0] == kind and cell in _cells(*t[1:])), None)

    def routes(self, peer, transfer):
        kind, r, _, _ = transfer
        row = r + HALF if kind in ("term", "relay") else r
        if self.middle:
            return [("AC".index(peer), row, row)]
        return [(0, _shifted(row), row), (1, row, row)]

    def remote(self, src, dst, send_sem, recv_slot, link):
        return pltpu.make_async_remote_copy(
            src, dst, send_sem, self.recv_sems.at[recv_slot],
            device_id=self.peers[link], device_id_type=pl.DeviceIdType.LOGICAL)

    def send(self, peer, transfer):
        kind, _, n, c = transfer
        slot = self.side * (self.recv_sems.shape[0] // 2) + self.links[self.role, peer].index(transfer)
        for link, here, at_middle in self.routes(peer, transfer):
            there = self.out_rows(here, n) if self.middle else pl.ds(at_middle, n)
            if kind == "x":
                src, dst = self.x.at[pl.ds(here, n)], self.x.at[there]
            elif kind == "final" or (peer, transfer) in self.totals:
                src = dst = self.out_tile(here, n, c)
            else:
                src = self.sums[self.summed[here, c]].at[c, pl.ds(here, n)]
                dst = self.inbox.at[self.side, c, there]
            self.sends.append(self.remote(src, dst, self.send_sems.at[len(self.sends)], slot, link))
            self.sends[-1].start()

    def receive(self, peer, transfer):
        if (peer, transfer) in self.arrived:
            return
        self.arrived.add((peer, transfer))
        kind, _, n, c = transfer
        total = kind == "final" or (self.role, transfer) in self.totals
        routes = self.routes(peer, transfer)
        for link, here, _ in routes:
            if kind == "x":
                dst = self.x.at[pl.ds(here, n)]
            else:
                dst = self.out_tile(here, n, c) if total else self.inbox.at[link, c, pl.ds(here, n)]
            slot = link * (self.recv_sems.shape[0] // 2) + self.links[peer, self.role].index(transfer)
            self.remote(dst, dst, self.send_sems.at[0], slot, link).wait_recv()
        if kind == "relay" and not total:
            for link, here, _ in routes:
                for cell in _cells(here, n, c):
                    self.put_total(link, *cell)

    def receive_tile(self, peer, kind, tile):
        for cell in _cells(*tile):
            transfer = self.carrier(peer, self.role, kind, cell)
            if transfer:
                self.receive(peer, transfer)

    def relay(self, end, tile):
        near = "AC".index(end)
        self.receive_tile("CA"[near], "term", tile)
        total = all((end, self.carrier(end, "M", "term", cell)) in self.arrived for cell in _cells(*tile))
        for r, c in _cells(tile[0] + HALF, *tile[1:]):
            if (r, c) not in self.summed:
                self.put_sum(near, r, c, self.own[c, pl.ds(r, CELL)] + self.received(1 - near, r, c))
            assert total or self.summed[r, c] == near
            if total and (r, c) not in self.complete:
                self.complete.add((r, c))
                self.put_total(self.summed[r, c], r, c)
        if total:
            self.totals.add((end, ("relay", *tile)))
        self.send(end, ("relay", *tile))

    def term(self, tile):
        self.receive_tile("M", "raw", tile)
        for row, c in _cells(*tile):
            for link, r in ((1, row), (0, row + HALF)):
                if (r, c) not in self.summed:
                    self.put_sum(0, r, c, self.own[c, pl.ds(r, CELL)] + self.received(link, r, c))
        self.send("M", ("term", *tile))

    def fence(self):
        pl.semaphore_signal(self.fence_sem, 1)
        pl.semaphore_wait(self.fence_sem, 1)

    def wait_sends(self, copies):
        self.fence()
        for copy in copies:
            copy.wait_send()
        self.fence()

    def run(self, text, barrier):
        for peer in self.peers:
            pl.semaphore_signal(barrier, 1, device_id=peer, device_id_type=pl.DeviceIdType.LOGICAL)
        started = []
        for line in text.strip().splitlines():
            for store in started:
                store()
            started = []
            for word in line.split():
                op, _, arg = word.lstrip("^").partition(":")
                if op[0] in "LW":
                    for name in [op[1:]] if op[1] == "x" else [op[1] + i for i in op[2:]]:
                        (self.load if op[0] == "L" else self.wait_load)(name)
                elif op == "enter":
                    pl.semaphore_wait(barrier, 2)
                elif op == "fence":
                    self.fence()
                elif op[0] in "khc":
                    blocks = [int(i) for i in op[1:]]
                    stores = ([self.output(c, arg) for c in blocks] if op[0] == "c"
                              else [self.hidden(op[0] == "k", blocks, arg)])
                    if word[0] == "^":
                        started += stores
                    else:
                        for store in stores:
                            store()
                elif op[0] == "x":
                    for r, n in _pieces(arg):
                        if op == "x>":
                            self.send("C" if self.middle else "M", ("x", r, n, None))
                        else:
                            self.receive(op[1], ("x", r, n, None))
                else:
                    for tile in _tiles(arg):
                        if op[0] == "<":
                            self.receive_tile(op[1], "term" if self.middle else "raw", tile)
                        elif op == "term":
                            self.term(tile)
                        elif op == "final":
                            self.receive_tile("M", "relay", tile)
                            self.send("M", ("final", *tile))
                        elif op[:-1] == "raw":
                            self.send(op[-1], ("raw", *tile))
                        else:
                            self.relay(op[-1], tile)
        assert not started
        rest = [(sender, t) for sender, receiver in self.links if receiver == self.role
                for t in self.links[sender, receiver] if (sender, t) not in self.arrived]
        self.wait_sends(self.sends[:-24])
        for sender, transfer in rest[:-1]:
            self.receive(sender, transfer)
        self.wait_sends(self.sends[-24:-2])
        self.wait_sends(self.sends[-2:])
        self.receive(*rest[-1])


def _mlp(schedule, x, W1, W2):
    links = _transfers(schedule)

    def body(*refs):
        w1_hbm, w1, load_sems = refs[1], refs[5], refs[-4]
        head = pl.ds(0, HEAD)
        pltpu.make_async_copy(w1_hbm.at[head], w1.at[head, pl.ds(0, H)], load_sems.at[0]).start()
        position = lax.axis_index("i")
        barrier = pltpu.get_barrier_semaphore()
        totals = set()
        for role, mine in (("M", (position & 1) == 1), ("C", position == 2), ("A", position == 0)):
            pl.when(mine)(lambda role=role: _Chip(role, position, links, totals, refs).run(schedule[role], barrier))

    longest = max(len(transfers) for transfers in links.values())
    blocks = N // LANES
    hbm = pl.BlockSpec(memory_space=pltpu.MemorySpace.HBM)
    return pl.pallas_call(
        body,
        out_shape=jax.ShapeDtypeStruct((M, N), jnp.bfloat16),
        in_specs=[hbm, hbm, hbm],
        out_specs=pl.BlockSpec(memory_space=pltpu.MemorySpace.VMEM),
        scratch_shapes=[
            pltpu.VMEM((M, K), jnp.float32),
            pltpu.VMEM((K, H + LANES), jnp.float32),
            [pltpu.VMEM((H // W2_RUN, W2_RUN, LANES), jnp.float32)] * blocks,
            pltpu.VMEM((M, K), jnp.bfloat16),
            pltpu.VMEM((M, H + LANES), jnp.float32),
            pltpu.VMEM((M, H), jnp.bfloat16),
            pltpu.VMEM((blocks, M, LANES), jnp.float32),
            [pltpu.VMEM((blocks, M, LANES), jnp.bfloat16)] * 2,
            pltpu.VMEM((2, blocks, M, LANES), jnp.bfloat16),
            pltpu.SemaphoreType.DMA((12,)),
            pltpu.SemaphoreType.DMA((2 * longest,)),
            pltpu.SemaphoreType.DMA((2 * longest,)),
            pltpu.SemaphoreType.REGULAR,
        ],
        compiler_params=pltpu.CompilerParams(
            collective_id=0,
            disable_bounds_checks=True,
            disable_semaphore_checks=True,
            flags={"XLA_TPU_RESCHEDULE_DMA_DONES": True},
        ),
    )(x, W1, W2.reshape(H // W2_RUN, W2_RUN, N))


def pallas_dist_mlp2_tp_i_m512_h1024_out512_kernel(
    x: jax.Array,
    W1: jax.Array,
    W2: jax.Array,
):
    return _mlp(SCHEDULE, x, W1, W2)
```
